```python
import numpy as np

kernel_name = "dist_matmul_relu_kshard_i_m1024_n1024_k512"

def setup_inputs():
    A = np.random.randn(1024, 2048).astype(np.float32)
    B = np.random.randn(2048, 1024).astype(np.float32)
    return {"A": A, "B": B}

def reference(A: np.ndarray, B: np.ndarray) -> np.ndarray:
    z = A @ B
    return np.maximum(z, 0.0)
```

```python
import jax
import jax.numpy as jnp
from jax import lax
from jax.experimental import pallas as pl
from jax.experimental.pallas import tpu as pltpu

M, N, K_SHARD = 1024, 1024, 512
Q = M // 4

CHUNKS = ((0, 128), (128, 128))
TAIL = 32
TILES = (
    (0, 64, 0, 128),
    (64, 64, 0, 128),
    (0, 64, 128, 128),
    (64, 64, 128, 128),
    (0, 128, 256, 128),
    (0, 128, 384, 256),
    (0, 128, 640, 384),
    (128, 128, 0, 1024),
)


def _new_operands():
    rows_seen, cols_seen, out = set(), set(), []
    for r0, nr, c0, nc in TILES:
        rows = [r for r in range(r0, r0 + nr) if r not in rows_seen]
        cols = [c for c in range(c0, c0 + nc) if c not in cols_seen]
        rows_seen.update(rows)
        cols_seen.update(cols)
        out.append(
            (
                (rows[0], len(rows)) if rows else None,
                (cols[0], len(cols)) if cols else None,
            )
        )
    return out


def _chunk_of(row):
    return next(c for c, (r0, nr) in enumerate(CHUNKS) if r0 <= row < r0 + nr)


def _kernel(
    a_hbm,
    b_hbm,
    out_ref,
    a_vmem,
    b_vmem,
    b_bf16,
    kept,
    send,
    recv,
    recv_sems,
):
    bf16, f32 = jnp.bfloat16, jnp.float32

    me = lax.axis_index("i")
    x = (me >> 1) & 1
    y = (me ^ (me >> 1)) & 1
    x_nbr, y_nbr = me ^ 3, me ^ 1
    first = (x_nbr, y_nbr)
    second = (y_nbr, x_nbr)
    keep = (x * Q, (2 + y) * Q)
    give = ((1 - x) * Q, (3 - y) * Q)

    def rows_at(base, r0, nr):
        return pl.ds(pl.multiple_of(base + r0, 16), nr)

    def wait_for_both_halves(step, sem, r0, nr):
        landed = recv.at[step, :, pl.ds(r0, nr)]
        pltpu.make_async_copy(landed, landed, recv_sems.at[step, sem]).wait()

    def write_received(r0, nr):
        for h in range(2):
            out_ref[rows_at(give[h], r0, nr), :] = recv[
                2, h, pl.ds(r0, nr), :
            ].astype(f32)

    def all_but_the_tail(load_sems, keep_sem, send_sem):
        def send_to(peer, step, h, sem, r0, nr, c0=0, nc=N):
            where = (step, h, pl.ds(r0, nr), pl.ds(c0, nc))
            pltpu.make_async_remote_copy(
                send.at[where],
                recv.at[where],
                send_sem,
                recv_sems.at[step, sem],
                device_id=(peer,),
                device_id_type=pl.DeviceIdType.MESH,
            ).start()

        loads = []
        for t, (rows, cols) in enumerate(_new_operands()):
            copies = []
            if cols:
                c = pl.ds(*cols)
                copies.append(
                    pltpu.make_async_copy(
                        b_hbm.at[:, c], b_vmem.at[:, c], load_sems.at[t]
                    )
                )
            if rows:
                copies += [
                    pltpu.make_async_copy(
                        a_hbm.at[rows_at(give[h], *rows)],
                        a_vmem.at[0, h, pl.ds(*rows)],
                        load_sems.at[t],
                    )
                    for h in range(2)
                ]
            for copy in copies:
                copy.start()
            loads.append((copies, cols))

        barrier = pltpu.get_barrier_semaphore()
        for nbr in (x_nbr, y_nbr):
            pl.semaphore_signal(
                barrier, 1, device_id=(nbr,), device_id_type=pl.DeviceIdType.MESH
            )

        keep_loads = [
            pltpu.make_async_copy(
                a_hbm.at[rows_at(keep[h], 0, Q)], a_vmem.at[1, h], keep_sem
            )
            for h in range(2)
        ]
        for copy in keep_loads:
            copy.start(priority=1)

        for t, ((r0, nr, c0, nc), (copies, cols)) in enumerate(zip(TILES, loads)):
            for copy in copies:
                copy.wait()
            if cols:
                c = pl.ds(*cols)
                b_bf16[:, c] = b_vmem[:, c].astype(bf16)
            a = jnp.concatenate(
                [a_vmem[0, h, pl.ds(r0, nr), :].astype(bf16) for h in range(2)]
            )
            part = jnp.dot(
                a, b_bf16[:, pl.ds(c0, nc)], preferred_element_type=f32
            ).astype(bf16)
            for h in range(2):
                send[0, h, pl.ds(r0, nr), pl.ds(c0, nc)] = part[h * nr : (h + 1) * nr]
            if t == 0:
                pl.semaphore_wait(barrier, 2)
            for h in range(2):
                send_to(first[h], 0, h, _chunk_of(r0), r0, nr, c0, nc)

        for copy in keep_loads:
            copy.wait()
        for r0, nr in CHUNKS:
            for h in range(2):
                kept[h, pl.ds(r0, nr), :] = jnp.dot(
                    a_vmem[1, h, pl.ds(r0, nr), :].astype(bf16),
                    b_bf16[...],
                    preferred_element_type=f32,
                )

        for c, (r0, nr) in enumerate(CHUNKS):
            wait_for_both_halves(0, c, r0, nr)
            r = pl.ds(r0, nr)
            for h in range(2):
                pair = kept[h, r, :] + recv[0, h, r, :].astype(f32)
                send[1, h, r, :] = pair.astype(bf16)
                send_to(second[h], 1, h, c, r0, nr)

        for c, (r0, nr) in enumerate(CHUNKS):
            wait_for_both_halves(1, c, r0, nr)
            r = pl.ds(r0, nr)
            for h in range(2):
                total = send[1, h, r, :].astype(f32) + recv[1, h, r, :].astype(f32)
                result = jnp.maximum(total, 0.0).astype(bf16)
                send[2, h, r, :] = result
                if c < len(CHUNKS) - 1:
                    send_to(first[h], 2, h, 0, r0, nr)
                else:
                    send_to(first[h], 2, h, 0, r0, nr - TAIL)
                    send_to(first[h], 2, h, 1, Q - TAIL, TAIL)
                out_ref[rows_at(keep[h], r0, nr), :] = result.astype(f32)

        wait_for_both_halves(2, 0, 0, Q - TAIL)
        write_received(0, Q - TAIL)
        pltpu.make_async_copy(send, send, send_sem).wait()

    pl.run_scoped(
        all_but_the_tail,
        pltpu.SemaphoreType.DMA((len(TILES),)),
        pltpu.SemaphoreType.DMA(()),
        pltpu.SemaphoreType.DMA(()),
    )
    wait_for_both_halves(2, 1, Q - TAIL, TAIL)
    write_received(Q - TAIL, TAIL)


def pallas_dist_matmul_relu_kshard_i_m1024_n1024_k512_kernel(
    A: jax.Array,
    B: jax.Array,
):
    return pl.pallas_call(
        _kernel,
        out_shape=jax.ShapeDtypeStruct((M, N), jnp.float32),
        in_specs=[pl.BlockSpec(memory_space=pl.ANY)] * 2,
        out_specs=pl.BlockSpec(memory_space=pltpu.VMEM),
        scratch_shapes=[
            pltpu.VMEM((2, 2, Q, K_SHARD), jnp.float32),
            pltpu.VMEM((K_SHARD, N), jnp.float32),
            pltpu.VMEM((K_SHARD, N), jnp.bfloat16),
            pltpu.VMEM((2, Q, N), jnp.float32),
            pltpu.VMEM((3, 2, Q, N), jnp.bfloat16),
            pltpu.VMEM((3, 2, Q, N), jnp.bfloat16),
            pltpu.SemaphoreType.DMA((3, 2)),
        ],
        compiler_params=pltpu.CompilerParams(
            collective_id=0, vmem_limit_bytes=32 * 1024 * 1024
        ),
    )(A, B)
```

```python
import jax
import jax.numpy as jnp
from jax import lax
from jax.experimental import pallas as pl
from jax.experimental.pallas import tpu as pltpu

M, N, K_SHARD = 1024, 1024, 512
Q = M // 4

CHUNKS = ((0, 128), (128, 128))
TAIL = 32
TILES = (
    (0, 64, 0, 128),
    (64, 64, 0, 128),
    (0, 64, 128, 128),
    (64, 64, 128, 128),
    (0, 128, 256, 128),
    (0, 128, 384, 256),
    (0, 128, 640, 384),
    (128, 128, 0, 1024),
)


def _new_operands():
    rows_seen, cols_seen, out = set(), set(), []
    for r0, nr, c0, nc in TILES:
        rows = [r for r in range(r0, r0 + nr) if r not in rows_seen]
        cols = [c for c in range(c0, c0 + nc) if c not in cols_seen]
        rows_seen.update(rows)
        cols_seen.update(cols)
        out.append(
            (
                (rows[0], len(rows)) if rows else None,
                (cols[0], len(cols)) if cols else None,
            )
        )
    return out


def _chunk_of(row):
    return next(c for c, (r0, nr) in enumerate(CHUNKS) if r0 <= row < r0 + nr)


def _kernel(
    a_hbm,
    b_hbm,
    out_ref,
    a_vmem,
    b_vmem,
    b_bf16,
    kept,
    send,
    recv,
    recv_sems,
):
    bf16, f32 = jnp.bfloat16, jnp.float32

    me = lax.axis_index("i")
    x = (me >> 1) & 1
    y = (me ^ (me >> 1)) & 1
    x_nbr, y_nbr = me ^ 3, me ^ 1
    first = (x_nbr, y_nbr)
    second = (y_nbr, x_nbr)
    keep = (x * Q, (2 + y) * Q)
    give = ((1 - x) * Q, (3 - y) * Q)

    def rows_at(base, r0, nr):
        return pl.ds(pl.multiple_of(base + r0, 16), nr)

    def wait_for_both_halves(step, sem, r0, nr):
        landed = recv.at[step, :, pl.ds(r0, nr)]
        pltpu.make_async_copy(landed, landed, recv_sems.at[step, sem]).wait()

    def write_received(r0, nr):
        for h in range(2):
            out_ref[rows_at(give[h], r0, nr), :] = recv[
                2, h, pl.ds(r0, nr), :
            ].astype(f32)

    def all_but_the_tail(load_sems, keep_sem, send_sem):
        def send_to(peer, step, h, sem, r0, nr, c0=0, nc=N):
            where = (step, h, pl.ds(r0, nr), pl.ds(c0, nc))
            pltpu.make_async_remote_copy(
                send.at[where],
                recv.at[where],
                send_sem,
                recv_sems.at[step, sem],
                device_id=(peer,),
                device_id_type=pl.DeviceIdType.MESH,
            ).start()

        loads = []
        for t, (rows, cols) in enumerate(_new_operands()):
            copies = []
            if cols:
                c = pl.ds(*cols)
                copies.append(
                    pltpu.make_async_copy(
                        b_hbm.at[:, c], b_vmem.at[:, c], load_sems.at[t]
                    )
                )
            if rows:
                copies += [
                    pltpu.make_async_copy(
                        a_hbm.at[rows_at(give[h], *rows)],
                        a_vmem.at[0, h, pl.ds(*rows)],
                        load_sems.at[t],
                    )
                    for h in range(2)
                ]
            for copy in copies:
                copy.start()
            loads.append((copies, cols))

        barrier = pltpu.get_barrier_semaphore()
        for nbr in (x_nbr, y_nbr):
            pl.semaphore_signal(
                barrier, 1, device_id=(nbr,), device_id_type=pl.DeviceIdType.MESH
            )

        keep_loads = [
            pltpu.make_async_copy(
                a_hbm.at[rows_at(keep[h], 0, Q)], a_vmem.at[1, h], keep_sem
            )
            for h in range(2)
        ]
        for copy in keep_loads:
            copy.start(priority=1)

        for t, ((r0, nr, c0, nc), (copies, cols)) in enumerate(zip(TILES, loads)):
            assert cols in (None, (c0, nc))
            for copy in copies:
                copy.wait()
            c = pl.ds(c0, nc)
            a = jnp.concatenate([a_vmem[0, h, pl.ds(r0, nr), :] for h in range(2)])
            b = b_vmem[:, c].astype(bf16) if cols else b_bf16[:, c]
            part = jnp.dot(a.astype(bf16), b, preferred_element_type=f32).astype(bf16)
            for h in range(2):
                send[0, h, pl.ds(r0, nr), c] = part[h * nr : (h + 1) * nr]
            if t == 0:
                pl.semaphore_wait(barrier, 2)
            for h in range(2):
                send_to(first[h], 0, h, _chunk_of(r0), r0, nr, c0, nc)
            if cols:
                b_bf16[:, c] = b_vmem[:, c].astype(bf16)

        for copy in keep_loads:
            copy.wait()
        for r0, nr in CHUNKS:
            for h in range(2):
                kept[h, pl.ds(r0, nr), :] = jnp.dot(
                    a_vmem[1, h, pl.ds(r0, nr), :].astype(bf16),
                    b_bf16[...],
                    preferred_element_type=f32,
                )

        for c, (r0, nr) in enumerate(CHUNKS):
            wait_for_both_halves(0, c, r0, nr)
            r = pl.ds(r0, nr)
            for h in range(2):
                pair = (kept[h, r, :] + recv[0, h, r, :].astype(f32)).astype(bf16)
                send[1, h, r, :] = pair
                send_to(second[h], 1, h, c, r0, nr)
                kept[h, r, :] = pair.astype(f32)

        for c, (r0, nr) in enumerate(CHUNKS):
            wait_for_both_halves(1, c, r0, nr)
            r = pl.ds(r0, nr)
            for h in range(2):
                total = kept[h, r, :] + recv[1, h, r, :].astype(f32)
                result = jnp.maximum(total, 0.0).astype(bf16)
                send[2, h, r, :] = result
                if c < len(CHUNKS) - 1:
                    send_to(first[h], 2, h, 0, r0, nr)
                else:
                    send_to(first[h], 2, h, 0, r0, nr - TAIL)
                    send_to(first[h], 2, h, 1, Q - TAIL, TAIL)
                out_ref[rows_at(keep[h], r0, nr), :] = result.astype(f32)

        wait_for_both_halves(2, 0, 0, Q - TAIL)
        write_received(0, Q - TAIL)
        pltpu.make_async_copy(send, send, send_sem).wait()

    pl.run_scoped(
        all_but_the_tail,
        pltpu.SemaphoreType.DMA((len(TILES),)),
        pltpu.SemaphoreType.DMA(()),
        pltpu.SemaphoreType.DMA(()),
    )
    wait_for_both_halves(2, 1, Q - TAIL, TAIL)
    write_received(Q - TAIL, TAIL)


def pallas_dist_matmul_relu_kshard_i_m1024_n1024_k512_kernel(
    A: jax.Array,
    B: jax.Array,
):
    return pl.pallas_call(
        _kernel,
        out_shape=jax.ShapeDtypeStruct((M, N), jnp.float32),
        in_specs=[pl.BlockSpec(memory_space=pl.ANY)] * 2,
        out_specs=pl.BlockSpec(memory_space=pltpu.VMEM),
        scratch_shapes=[
            pltpu.VMEM((2, 2, Q, K_SHARD), jnp.float32),
            pltpu.VMEM((K_SHARD, N), jnp.float32),
            pltpu.VMEM((K_SHARD, N), jnp.bfloat16),
            pltpu.VMEM((2, Q, N), jnp.float32),
            pltpu.VMEM((3, 2, Q, N), jnp.bfloat16),
            pltpu.VMEM((3, 2, Q, N), jnp.bfloat16),
            pltpu.SemaphoreType.DMA((3, 2)),
        ],
        compiler_params=pltpu.CompilerParams(
            collective_id=0, vmem_limit_bytes=32 * 1024 * 1024
        ),
    )(A, B)
```
